```python
import numpy as np

kernel_name = "dist_sparse_attn_causalblk_htp_bs_b2_sq256_skv256_hq4_dh64"

def setup_inputs():
    x = np.random.randn(8, 256, 512).astype(np.float32)
    Wq = np.random.randn(512, 1024).astype(np.float32) * 0.02
    K_ext = np.random.randn(8, 256, 16, 64).astype(np.float32)
    V_ext = np.random.randn(8, 256, 16, 64).astype(np.float32)
    Wo = np.random.randn(1024, 512).astype(np.float32) * 0.02
    return {"x": x, "Wq": Wq, "K_ext": K_ext, "V_ext": V_ext, "Wo": Wo}

def reference(x, Wq, K_ext, V_ext, Wo):
    B, Sq, Skv, Hq, Dh = 8, 256, 256, 16, 64
    Q = (x @ Wq).reshape(B, Sq, Hq, Dh)
    qb = (np.arange(Sq) // 64)[:, None]
    kb = (np.arange(Skv) // 64)[None, :]
    mask = kb <= qb
    scores = np.einsum('bihd,bjhd->bhij', Q, K_ext).astype(np.float32) * 0.125
    scores = np.where(mask[None, None, :, :], scores, -1e9)
    scores_max = scores.max(axis=-1, keepdims=True)
    w = np.exp(scores - scores_max)
    row_keep = mask.any(axis=1)
    w_sum = np.where(row_keep[None, None, :, None], w.sum(axis=-1, keepdims=True), 1.0)
    w = w / w_sum
    w = np.where(row_keep[None, None, :, None], w, 0.0)
    ctx = np.einsum('bhij,bjhd->bihd', w, V_ext).reshape(B, Sq, Hq * Dh)
    return ctx @ Wo
```

```python
import contextlib
import math

import jax
import jax.numpy as jnp
from jax import lax
from jax.experimental import pallas as pl
from jax.experimental.pallas import tpu as pltpu

B_LOC, SQ, D_MODEL = 2, 256, 512
ROWS = B_LOC * SQ
BLK = 64
NBLK = SQ // BLK
SCALE = 0.125 * math.log2(math.e)
MESH = pl.DeviceIdType.MESH
BF16, F32, I32 = jnp.bfloat16, jnp.float32, jnp.int32
QA, QB, OA, QC, OB, OC = range(6)


def make(scopes=False, asym=True, wq_chunks=(32, 96, 384), tail=(4, 2, 1, 1), nocheck=True, nobounds=False):
    def scope(name):
        return jax.named_scope(name) if scopes else contextlib.nullcontext()

    NQ = len(wq_chunks)

    def body(x_hbm, wq_hbm, kt_hbm, vt_hbm, wo_hbm, out_ref,
             xf, wqf, wof, kvf, xb, tx, rx, kvb, ctx, acc,
             ld_sem, send_sem, recv_sem, go_sem):
        me = lax.axis_index("i")
        nbr = (me ^ 1, me ^ 3)
        diag = me ^ 2
        barrier = pltpu.get_barrier_semaphore()

        starts = [sum(wq_chunks[:i]) for i in range(NQ)]
        ld_wq = [pltpu.make_async_copy(wq_hbm.at[pl.ds(s, n)], wqf.at[pl.ds(s, n)], ld_sem.at[i])
                 for i, (s, n) in enumerate(zip(starts, wq_chunks))]
        for c in ld_wq:
            c.start()

        def hello():
            for n in nbr:
                pl.semaphore_signal(barrier, inc=1, device_id=(n,), device_id_type=MESH)
        if asym:
            pl.when(me != 2)(hello)
        else:
            hello()

        ld_x = pltpu.make_async_copy(x_hbm, xf, ld_sem.at[NQ])
        ld_wo = pltpu.make_async_copy(wo_hbm, wof, ld_sem.at[NQ + 1])
        owners = ((me, me), (nbr[0], nbr[1]), (nbr[1], nbr[0]), (diag, diag))

        def ld_kv(g):
            for p in range(2):
                rows = pl.ds(pl.multiple_of(owners[g][p] * 256 + p * 128, 128), 128)
                for b in range(B_LOC):
                    for t, src in enumerate((kt_hbm, vt_hbm)):
                        pltpu.make_async_copy(src.at[me * B_LOC + b, rows], kvf.at[g, 2 * p + b, t],
                                              ld_sem.at[NQ + 2 + g]).start()

        ld_wo.start()
        ld_x.start()
        ld_kv(0)

        def send(src, stage, part, d, rows=slice(None), sem=None):
            pltpu.make_async_remote_copy(
                src.at[rows], rx.at[stage, part, rows], send_sem, recv_sem.at[stage if sem is None else sem],
                device_id=(nbr[d],), device_id_type=MESH).start()

        def recv(stage, rows=slice(None), sem=None):
            r = rx.at[stage, :, rows]
            pltpu.make_async_copy(r, r, recv_sem.at[stage if sem is None else sem]).wait()

        with scope("barrier"):
            if asym:
                @pl.when((me & 1) == 1)
                def _():
                    pl.semaphore_wait(barrier, 1)

                @pl.when((me & 1) == 0)
                def _():
                    pl.semaphore_wait(barrier, 2)

                @pl.when(me == 2)
                def _():
                    for n_ in nbr:
                        pl.semaphore_signal(go_sem, inc=1, device_id=(n_,), device_id_type=MESH)
            else:
                pl.semaphore_wait(barrier, 2)
        late = (me == 3, me == 1)
        for i, (s, n) in enumerate(zip(starts, wq_chunks)):
            with scope("ld_wq"):
                ld_wq[i].wait()
                rows = slice(s, s + n)
                for p in range(2):
                    tx[p, rows] = wqf[rows, p * 128:(p + 1) * 128].astype(BF16)
            for d in range(2):
                def first(d=d):
                    send(tx.at[d], QA, d, d, rows)
                    if i == NQ - 1:
                        send(tx.at[1 - d], QB, 1 - d, d)
                if asym:
                    pl.when(jnp.logical_not(late[d]))(first)
                else:
                    first()
        if asym:
            with scope("go"):
                for d in range(2):
                    @pl.when(late[d])
                    def _():
                        pl.semaphore_wait(go_sem, 1)
                        send(tx.at[d], QA, d, d)
                        send(tx.at[1 - d], QB, 1 - d, d)

        def ldi(ref):
            return ref.bitcast(I32)[...]

        def bf(v):
            return pltpu.bitcast(v, BF16)

        def ld(ref):
            return bf(ldi(ref))

        lo32 = lax.broadcasted_iota(I32, (BLK // 2, 128), 1) < BLK
        lo = lax.broadcasted_iota(I32, (BLK, 128), 1) < BLK

        def attend(g, w):
            st = {}

            def blockdiag(u, t):
                out = []
                for h in range(2):
                    v = kvf[g, u, t, :, h * 128:(h + 1) * 128]
                    if t == 0:
                        v = v * SCALE
                    kvb[g, u, t, h] = v.astype(BF16)
                    v = ldi(kvb.at[g, u, t, h])
                    top, bot = v[:32], v[32:]
                    r = pltpu.roll(jnp.where(lo32, bot, top), BLK, 1)
                    z = jnp.zeros_like(top)
                    out.append(bf(jnp.concatenate([jnp.where(lo32, top, z), jnp.where(lo32, z, r)], 0)))
                    out.append(bf(jnp.concatenate([jnp.where(lo32, r, z), jnp.where(lo32, z, bot)], 0)))
                return out

            def q_proj(u):
                p, b = divmod(u, 2)
                xs = jnp.concatenate([ld(xb.at[k, b * SQ:(b + 1) * SQ]) for k in range(4)], 1)
                st["q", u] = jnp.dot(xs, w(p), preferred_element_type=F32).astype(BF16)

            def scores(u):
                k = blockdiag(u, 0)
                st["s", u] = [jnp.dot(st["q", u][j * BLK:], k[j], preferred_element_type=F32)
                              for j in range(NBLK)]

            def softmax(u):
                pr = [[None] * NBLK for _ in range(NBLK)]
                inv = []
                for i in range(NBLK):
                    blocks = [st["s", u][j][(i - j) * BLK:(i - j + 1) * BLK] for j in range(i + 1)]
                    m = blocks[0]
                    for t in blocks[1:]:
                        m = jnp.maximum(m, t)
                    m0 = jnp.max(jnp.where(lo, m, -jnp.inf), axis=1, keepdims=True)
                    m1 = jnp.max(jnp.where(lo, -jnp.inf, m), axis=1, keepdims=True)
                    m = jnp.where(lo, m0, m1)
                    tot = None
                    for j in range(i + 1):
                        e = jnp.exp2(blocks[j] - m)
                        tot = e if tot is None else tot + e
                        pr[j][i] = e.astype(BF16)
                    l0 = jnp.sum(jnp.where(lo, tot, 0.0), axis=1, keepdims=True)
                    l1 = jnp.sum(jnp.where(lo, 0.0, tot), axis=1, keepdims=True)
                    inv.append(pl.reciprocal(jnp.where(lo, l0, l1), approx=True))
                st["p", u], st["inv", u] = pr, inv

            def context(u):
                p, b = divmod(u, 2)
                v = blockdiag(u, 1)
                o = [lax.dot_general(jnp.concatenate(st["p", u][j][j:], 0), v[j],
                                     (((1,), (1,)), ((), ())), preferred_element_type=F32)
                     for j in range(NBLK)]
                for i in range(NBLK):
                    t = o[0][i * BLK:(i + 1) * BLK]
                    for j in range(1, i + 1):
                        t = t + o[j][(i - j) * BLK:(i - j + 1) * BLK]
                    r0 = b * SQ + i * BLK
                    ctx[g, p, r0:r0 + BLK, :] = (t * st["inv", u][i]).astype(BF16)

            q_proj(0)
            q_proj(1)
            pltpu.make_async_copy(kvf.at[g], kvf.at[g], ld_sem.at[NQ + 2 + g]).wait()
            for t in range(5):
                if t < 4:
                    scores(t)
                if t + 2 < 4:
                    q_proj(t + 2)
                if t < 4:
                    softmax(t)
                if t > 0:
                    context(t - 1)

        lo256 = lax.broadcasted_iota(I32, (ROWS // 2, 128), 1) < BLK

        def project(terms, tiles, first=False, last=False, split=1):
            n = ROWS // split
            for c in sorted({k // 2 for k in tiles}):
                ks = [k for k in tiles if k // 2 == c]
                for r in range(split):
                    a, w = [], []
                    for lhs, top, bot in terms:
                        for k in ks:
                            rows = slice(k * BLK, (k + 1) * BLK)
                            w += [ld(top.at[rows]), ld(bot.at[rows])]
                            a.append(bf(lhs(k % 2)[r * n // 2:(r + 1) * n // 2]))
                    t = jnp.dot(jnp.concatenate(a, 1), jnp.concatenate(w, 0), preferred_element_type=F32)
                    idx = (slice(r * n, (r + 1) * n), slice(c * 128, (c + 1) * 128))
                    if not first:
                        t = t + acc[idx]
                    if last and ks[-1] % 2 == 1:
                        out_ref[idx] = t.astype(out_ref.dtype)
                    else:
                        acc[idx] = t

        with scope("ld_wo"):
            ld_wo.wait()
            ld_kv(1)
            for h in range(2):
                for k in range(8):
                    r0, c = (k % 2) * 128 + h * BLK, k // 2
                    tx[2 + h, k * BLK:(k + 1) * BLK] = wof[r0:r0 + BLK, c * 128:(c + 1) * 128].astype(BF16)
            for d in range(2):
                send(tx.at[2 + d], OA, d, d)
        with scope("ld_x"):
            ld_x.wait()
            ld_kv(2)
            for k in range(4):
                xb[k] = xf[:, k * 128:(k + 1) * 128].astype(BF16)
        with scope("att_own"):
            attend(0, lambda p: ld(tx.at[p]))
        with scope("w_a"):
            ld_kv(3)
            recv(QA)
            for d in range(2):
                send(rx.at[QA, 1 - d], QC, 1 - d, d)
            for d in range(2):
                send(tx.at[3 - d], OB, 1 - d, d)
        with scope("att_a"):
            attend(1, lambda p: ld(rx.at[QA, p]))
        with scope("w_b"):
            recv(QB)
        with scope("att_b"):
            attend(2, lambda p: ld(rx.at[QB, p]))
        t0 = [sum(tail[:i]) for i in range(len(tail))]
        with scope("w_d"):
            recv(OA)
            for i, (s, n) in enumerate(zip(t0, tail)):
                for d in range(2):
                    send(rx.at[OA, 1 - d], OC, 1 - d, d, slice(s * BLK, (s + n) * BLK), OC + i)
        with scope("proj_d"):
            project([(lambda p: ldi(ctx.at[0, p]), tx.at[2], tx.at[3]),
                     (lambda p: jnp.where(lo256, ldi(ctx.at[1 + p, p]), ldi(ctx.at[2 - p, p])),
                      rx.at[OA, 0], rx.at[OA, 1])], range(8), first=True)
        with scope("w_c"):
            recv(QC)
        with scope("att_c"):
            attend(3, lambda p: ld(rx.at[QC, p]))
        with scope("w_e"):
            recv(OB)
        with scope("proj_e"):
            project([(lambda p: jnp.where(lo256, ldi(ctx.at[2 - p, p]), ldi(ctx.at[1 + p, p])),
                      rx.at[OB, 0], rx.at[OB, 1])], range(8))
        for i, (s, n) in enumerate(zip(t0, tail)):
            with scope("w_f"):
                recv(OC, slice(s * BLK, (s + n) * BLK), OC + i)
            with scope("proj_f"):
                project([(lambda p: ldi(ctx.at[3, p]), rx.at[OC, 0], rx.at[OC, 1])], range(s, s + n), last=True,
                        split=max(1, 4 // n))
        with scope("w_send"):
            pltpu.make_async_copy(rx, rx, send_sem).wait()

    def kernel(x, Wq, K_ext, V_ext, Wo):
        kt = jnp.transpose(K_ext, (0, 2, 3, 1)).reshape(8, 1024, SQ)
        vt = jnp.transpose(V_ext, (0, 2, 3, 1)).reshape(8, 1024, SQ)
        hbm = pl.BlockSpec(memory_space=pltpu.HBM)
        out = pl.pallas_call(
            body,
            out_shape=jax.ShapeDtypeStruct((ROWS, D_MODEL), BF16),
            in_specs=[hbm] * 5,
            out_specs=pl.BlockSpec(memory_space=pltpu.VMEM),
            scratch_shapes=[
                pltpu.VMEM((ROWS, D_MODEL), F32),
                pltpu.VMEM((D_MODEL, 256), F32),
                pltpu.VMEM((256, D_MODEL), F32),
                pltpu.VMEM((4, 4, 2, 128, SQ), F32),
                pltpu.VMEM((4, ROWS, 128), BF16),
                pltpu.VMEM((4, 512, 128), BF16),
                pltpu.VMEM((6, 2, 512, 128), BF16),
                pltpu.VMEM((4, 4, 2, 2, 128, 128), BF16),
                pltpu.VMEM((4, 2, ROWS, 128), BF16),
                pltpu.VMEM((ROWS, D_MODEL), F32),
                pltpu.SemaphoreType.DMA((NQ + 6,)),
                pltpu.SemaphoreType.DMA,
                pltpu.SemaphoreType.DMA((OC + len(tail),)),
                pltpu.SemaphoreType.REGULAR,
            ],
            compiler_params=pltpu.CompilerParams(collective_id=0, vmem_limit_bytes=48 << 20,
                                                 disable_semaphore_checks=nocheck,
                                                 disable_bounds_checks=nobounds),
        )(x.reshape(ROWS, D_MODEL), Wq, kt, vt, Wo)
        return out.reshape(B_LOC, SQ, D_MODEL)

    return kernel


pallas_dist_sparse_attn_causalblk_htp_bs_b2_sq256_skv256_hq4_dh64_kernel = make(nocheck=False)
```

```python
import math

import jax
import jax.numpy as jnp
from jax import lax
from jax.experimental import pallas as pl
from jax.experimental.pallas import tpu as pltpu

BF16, F32, I32 = jnp.bfloat16, jnp.float32, jnp.int32
MESH = pl.DeviceIdType.MESH
NB, SEQ, D_MODEL = 2, 256, 512
BLK = 64
NBLK = SEQ // BLK
SCALE = 0.125 * math.log2(math.e)

CODE, BITS, RAW, END = 0, 48, 176, 264
_srl = lax.shift_right_logical
_EXP = 0x7F807F80
_HOME, _TAIL = 96, 192
_WORDS = [5] * 4 + [4] * 4 + [3] * 4 + [2] * 3 + [1]


def _bytes(b):
    v = b * 0x01010101
    return v - (1 << 32) if v >> 31 else v


def _splat(v):
    v = v | (v << 8)
    return v | (v << 16)


def _sign_mantissa(w0, w1):
    return (w0 & ~_EXP) | (((w1 << 8) | _srl(w1, 24)) & _EXP)


def _exponents(w0, w1):
    return (_srl(w0, 7) & 0x00FF00FF) | ((w1 << 1) & ~0x00FF00FF)


def _join(sm, e):
    return [(sm & ~_EXP) | ((e << 7) & _EXP),
            ((_srl(sm, 8) | (sm << 24)) & ~_EXP) | (_srl(e, 1) & _EXP)]


def _below(v, k):
    return _srl(_bytes(127 + (1 << k)) - v, 7) & _bytes(1)


def _rot_up(v, k):
    t = _below(v, k)
    return (v + t) & ~(t << k)


def _rot_down(v, k):
    t = _below(v, k)
    return ((v | (t << k)) - t) & ~(t << k)


def _encode(w):
    row = lax.broadcasted_iota(I32, (8, 128), 0)

    def over_rows(op, v):
        for n in (1, 2, 4):
            v = op(v, pltpu.roll(v, n, 0))
        return v

    big, tot = None, 0
    for v in w:
        m = jnp.maximum(pltpu.bitcast((v << 16) & 0x7F800000, F32),
                        pltpu.bitcast(v & 0x7F800000, F32))
        big = m if big is None else jnp.maximum(big, m)
        tot = tot + (_srl(v, 7) & 0x00FF00FF)
    tot = over_rows(jnp.add, tot)
    top = _srl((tot & 0xFFFF) + _srl(tot, 16) + 1856, 9)
    top = jnp.maximum(_srl(pltpu.bitcast(over_rows(jnp.maximum, big), I32), 23), top)
    top = jnp.minimum(top, 255)
    top4 = _splat(top)

    e = [_exponents(w[2 * k], w[2 * k + 1]) for k in range(16)]
    odd, bad, groups = [0, 0], 0, []
    for k in range(16):
        d = top4 - e[k]
        bad |= d & _bytes(0xC0)
        u = _rot_down(_rot_down(d, 3), 2)
        odd[k // 8] |= (u & _bytes(1)) << (k % 8)
        stop = _srl(u, 1) & _bytes(31)
        stop = stop + 0x01010100
        stop = stop + (stop << 8)
        stop = stop + (stop << 16)
        bits = 0
        for b in range(4):
            bits |= 1 << (_srl(stop, 8 * b) & 31)
        n = _srl(stop, 24) + 1
        bad |= n & ~31
        groups.append((bits, n & 31))

    stream, total = [groups[15][0]], groups[15][1]
    for k in range(14, -1, -1):
        bits, n = groups[k]
        if _WORDS[k] > _WORDS[k + 1]:
            bad |= (32 * _WORDS[k + 1] - total) & ~255
        back = (32 - n) & 31
        stream = ([(stream[0] << n) | bits]
                  + [(a << n) | _srl(b, back) for a, b in zip(stream[1:], stream)]
                  + [_srl(stream[-1], back)])[:_WORDS[k]]
        total = total + n

    over = jnp.maximum(total - _HOME, 0)
    end = over
    for n in (1, 2, 4):
        end = end + jnp.where(row >= n, pltpu.roll(end, n, 0), 0)
    misfit = (bad != 0) | (total > 32 * _WORDS[0]) | (end > _TAIL)
    misfit = jnp.max(jnp.where(misfit, 1.0, 0.0)) > 0.5
    off = end - over
    n = off & 31
    x = ([stream[0] << n]
         + [(a << n) | _srl(_srl(b, 1), 31 - n) for a, b in zip(stream[1:], stream)]
         + [_srl(_srl(stream[-1], 1), 31 - n)])
    for step in (1, 2, 4):
        move = (off & (32 * step)) != 0
        x = [jnp.where(move, a, b) for a, b in zip([0] * step + x, x + [0] * step)]
    home, tail = [], 0
    for j in range(3):
        h, t = x[j], 0
        for m in (1, 2, 3):
            r = pltpu.roll(x[j + 3 * m], m, 0)
            h, t = h | jnp.where(row < m, 0, r), t | jnp.where(row < min(m, 2), r, 0)
        home.append(h)
        tail |= pltpu.roll(t, 2 * j, 0) if j else t
    head = jnp.where(row == 0, top, off & 255) << (_srl(row, 1) << 3)
    for n in (2, 4):
        head |= pltpu.roll(head, n, 0)
    return e, odd + home + [jnp.where(row >= 6, head, tail)], misfit


def _decode(code):
    row = lax.broadcasted_iota(I32, (8, 128), 0)
    odd, home, tail = code[:2], code[2:5], code[5]
    head = jnp.where(row >= 6, tail, 0)
    for n in (2, 4):
        head |= pltpu.roll(head, n, 0)
    off = jnp.where(row == 0, 0, _srl(head, _srl(row, 1) << 3))
    top4 = _splat(jnp.where((row & 1) == 0, head, pltpu.roll(head, 1, 0)) & 255)
    x = list(home)
    for m in (1, 2, 3):
        for j in range(3):
            t = pltpu.roll(tail, 8 - 2 * j, 0) if j else tail
            x.append(pltpu.roll(jnp.where(row < m, t, home[j]), 8 - m, 0))
    for step in (4, 2, 1):
        move = (off & (32 * step)) != 0
        x = [jnp.where(move, x[min(i + step, len(x) - 1)], x[i]) for i in range(5 + step)]
    n = off & 31
    stream = [_srl(a, n) | ((b << 1) << (31 - n)) for a, b in zip(x, x[1:])]
    e = []
    for k in range(16):
        v, stop = stream[0], 0
        for b in range(4):
            rest = v & (v - 1)
            f = pltpu.bitcast((v - rest).astype(F32), I32)
            stop |= _srl(f, 23 - 8 * b) if b < 3 else f << 1
            v = rest
        u = ((stop - (stop << 8) - 0x0101017F) << 1) | (_srl(odd[k // 8], k % 8) & _bytes(1))
        e.append(top4 - _rot_up(_rot_up(u, 2), 3))
        if k < 15:
            n = (_srl(f, 23) + 2) & 31
            back = (32 - n) & 31
            stream = ([_srl(a, n) | (b << back) for a, b in zip(stream, stream[1:])]
                      + [_srl(stream[-1], n)])[:_WORDS[k + 1]]
    return e


QA, QB, QC, OA, OB, OC = range(6)
_WQ_ROWS = (0, 32, 64, 128, 192, 256, 384, 512)
_PIECES = ((QA, 0, 8), (QB, 0, 8), (QC, 0, 8), (OA, 0, 2), (OA, 2, 8), (OB, 0, 6), (OB, 6, 8),
           (OC, 0, 2), (OC, 2, 4), (OC, 4, 6), (OC, 6, 8))
_N_WQ = len(_WQ_ROWS) - 1


def _pack(v):
    return pltpu.bitcast(v.astype(BF16), I32)


def _bf16(v):
    return pltpu.bitcast(v, BF16)


def _tiles(v):
    return [v[i:i + 8] for i in range(0, v.shape[0], 8)]


def _unit(u):
    g, r = divmod(u, 4)
    return (g, r % 2, r // 2) if g == 0 else (g, r // 2, r % 2)


def _body(x_hbm, wq_hbm, kt_hbm, vt_hbm, wo_hbm, out_ref,
          x_f32, wq_f32, wo_f32, kv_f32, xs, own, tx, rx, ctx, acc,
          load_sem, send_sem, recv_sem, go_sem):
    me = lax.axis_index("i")
    nbr = (me ^ 1, me ^ 3)
    head_owner = ((me, me), (nbr[0], nbr[1]), (nbr[1], nbr[0]), (me ^ 2, me ^ 2))

    load_wq = [pltpu.make_async_copy(wq_hbm.at[a:b], wq_f32.at[a:b], load_sem.at[i])
               for i, (a, b) in enumerate(zip(_WQ_ROWS, _WQ_ROWS[1:]))]
    load_x = [pltpu.make_async_copy(x_hbm.at[b], x_f32.at[b], load_sem.at[_N_WQ + b])
              for b in range(NB)]
    load_wo = pltpu.make_async_copy(wo_hbm, wo_f32, load_sem.at[_N_WQ + 2])

    def load_kv(*pairs):
        for h in pairs:
            for u in (2 * h, 2 * h + 1):
                g, p, b = _unit(u)
                rows = pl.ds(pl.multiple_of(head_owner[g][p] * 256 + p * 128, 128), 128)
                for t, src in enumerate((kt_hbm, vt_hbm)):
                    pltpu.make_async_copy(src.at[me * NB + b, rows], kv_f32.at[u, t],
                                          load_sem.at[_N_WQ + 3 + h]).start()

    def wait_kv(*pairs):
        for h in pairs:
            r = kv_f32.at[2 * h:2 * h + 2]
            pltpu.make_async_copy(r, r, load_sem.at[_N_WQ + 3 + h]).wait()

    verbatim, raw_sends = {}, []

    def route(stage, d):
        part = d if stage % 3 == 0 else 1 - d
        if stage % 3 == 2:
            return part, rx.at[stage - 2, part], (stage - 2, part)
        m = 2 * (stage // 3) + part
        return part, tx.at[m], m

    def copy(stage, d, a, b, recv, send=0):
        part, src, _ = route(stage, d)
        return pltpu.make_async_remote_copy(
            src.at[a:b], rx.at[stage, part, a:b], send_sem.at[send], recv_sem.at[recv],
            device_id=(nbr[d],), device_id_type=MESH)

    def bits_sem(*piece):
        return 18 + _PIECES.index(piece)

    def send_bits(*pieces):
        for stage, a, b in pieces:
            for d in range(2):
                copy(stage, d, BITS + 16 * a, BITS + 16 * b, bits_sem(stage, a, b)).start()

    def recv_bits(*pieces):
        for stage, a, b in pieces:
            r = rx.at[stage, :, BITS + 16 * a:BITS + 16 * b]
            pltpu.make_async_copy(r, r, recv_sem.at[bits_sem(stage, a, b)]).wait()

    def send_raw(stage):
        for d in range(2):
            part, _, key = route(stage, d)
            cp = copy(stage, d, RAW, END, 2 * stage + part, 1 + 2 * stage + part)
            pl.when(verbatim[key])(cp.start)
            raw_sends.append((verbatim[key], cp))

    def recv_raw(stage):
        for part in range(2):
            r = rx.at[stage, part, RAW:END]
            pl.when(verbatim[stage, part])(
                pltpu.make_async_copy(r, r, recv_sem.at[2 * stage + part]).wait)
        if stage % 3 == 0:
            send_raw(stage + 2)

    def send_code(stage):
        for d in range(2):
            copy(stage, d, CODE, BITS, 12 + stage).start()
        if stage % 3 < 2:
            send_raw(stage)

    def recv_code(stage):
        r = rx.at[stage, :, CODE:BITS]
        pltpu.make_async_copy(r, r, recv_sem.at[12 + stage]).wait()

    def put_bits(m, a, b):
        w = _tiles(own[m, a:b])
        for k in range(len(w) // 2):
            r = BITS + a // 2 + 8 * k
            tx[m, r:r + 8] = _sign_mantissa(w[2 * k], w[2 * k + 1])

    def put_code(m):
        e, code, verbatim[m] = _encode(_tiles(own[m]))
        tx[m, CODE:BITS] = jnp.concatenate(
            [jnp.where(verbatim[m], a, b) for a, b in zip(e[:5] + [-1], code)], 0)
        tx[m, RAW:END] = jnp.concatenate(e[5:], 0)

    exps = {}

    def read_code(stage):
        return [[rx[stage, part, r:r + 8] for r in range(CODE + 16, BITS, 8)] for part in range(2)]

    def decode(stage, rest):
        for part in range(2):
            verbatim[stage, part] = rest[part][-1][7, 0] == -1
            exps[stage, part] = _decode(_tiles(rx[stage, part, CODE:CODE + 16]) + rest[part])

    def received(stage, part, k0, k1):
        msg = rx.at[stage, part]
        marker = jnp.broadcast_to(msg[BITS - 1:BITS], (8, 128)) == -1
        out = []
        for k in range(k0, k1):
            r = CODE + 8 * k if k < 5 else RAW + 8 * (k - 5)
            e = jnp.where(marker, msg[r:r + 8], exps[stage, part][k])
            out += _join(msg[BITS + 8 * k:BITS + 8 * k + 8], e)
        return _bf16(jnp.concatenate(out, 0))

    first = lax.broadcasted_iota(I32, (BLK, 128), 1) < BLK
    wq, q, prob, inv = {}, {}, {}, {}

    def block_diag(u, t):
        out = []
        for h in range(2):
            v = kv_f32[u, t, :, h * 128:(h + 1) * 128]
            if t == 0:
                v = v * SCALE
            h0, h1 = v[:BLK], v[BLK:]
            r = pltpu.roll(jnp.where(first, h1, h0), BLK, 1)
            for a, b in ((h0, r), (r, h1)):
                out.append(jnp.concatenate(
                    [jnp.where(first, a, 0.0), jnp.where(first, 0.0, b)], 0).astype(BF16))
        return out

    def query(*units):
        for u in units:
            g, p, b = _unit(u)
            if g == 0:
                wq[g, p] = _bf16(own[p])
            elif b == 0:
                wq[g, p] = received(g - 1, p, 0, 16)
            lhs = jnp.concatenate([_bf16(xs[b, k]) for k in range(4)], 1)
            q[u] = jnp.dot(lhs, wq[g, p], preferred_element_type=F32)

    def softmax(*units):
        for u in units:
            k = block_diag(u, 0)
            s = [jnp.dot(q[u][j * BLK:].astype(BF16), k[j], preferred_element_type=F32)
                 for j in range(NBLK)]
            w, inv[u] = [[] for _ in range(NBLK)], []
            for i in range(NBLK):
                blocks = [s[j][(i - j) * BLK:(i - j + 1) * BLK] for j in range(i + 1)]
                m = blocks[0]
                for t in blocks[1:]:
                    m = jnp.maximum(m, t)
                m = jnp.where(first,
                              jnp.max(jnp.where(first, m, -jnp.inf), axis=1, keepdims=True),
                              jnp.max(jnp.where(first, -jnp.inf, m), axis=1, keepdims=True))
                tot = None
                for j in range(i + 1):
                    e = jnp.exp2(blocks[j] - m)
                    tot = e if tot is None else tot + e
                    w[j].append(e)
                tot = jnp.where(first,
                                jnp.sum(jnp.where(first, tot, 0.0), axis=1, keepdims=True),
                                jnp.sum(jnp.where(first, 0.0, tot), axis=1, keepdims=True))
                inv[u].append(pl.reciprocal(tot, approx=True))
            prob[u] = [jnp.concatenate(t, 0).astype(BF16) for t in w]

    def context(*units):
        for u in units:
            g, p, b = _unit(u)
            v = block_diag(u, 1)
            o = [lax.dot_general(prob[u][j], v[j], (((1,), (1,)), ((), ())),
                                 preferred_element_type=F32) for j in range(NBLK)]
            for i in range(NBLK):
                t = o[0][i * BLK:(i + 1) * BLK]
                for j in range(1, i + 1):
                    t = t + o[j][(i - j) * BLK:(i - j + 1) * BLK]
                ctx[g, p, b, i * 32:(i + 1) * 32] = _pack(t * inv[u][i])

    def project_own(b, *cols):
        for c in cols:
            rhs = [_bf16(own[2 + h, 64 * c + 32 * p:64 * c + 32 * p + 32])
                   for p in range(2) for h in range(2)]
            for r in (0, 128):
                lhs = [_bf16(ctx[0, p, b, r // 2:r // 2 + 64]) for p in range(2)]
                acc[b, r:r + 128, c * 128:(c + 1) * 128] = jnp.dot(
                    jnp.concatenate(lhs, 1), jnp.concatenate(rhs, 0), preferred_element_type=F32)

    def project(stage, *cols):
        def heads(p, b):
            if stage == OC:
                return ctx[3, p, b]
            g0, g1 = (1 + p, 2 - p) if stage == OA else (2 - p, 1 + p)
            return jnp.where(lax.broadcasted_iota(I32, (SEQ // 2, 128), 1) < BLK,
                             ctx[g0, p, b], ctx[g1, p, b])

        for c in cols:
            rhs = [received(stage, h, 4 * c + 2 * p, 4 * c + 2 * p + 2)
                   for p in range(2) for h in range(2)]
            for b in range(NB):
                lhs = [_bf16(heads(p, b)) for p in range(2)]
                t = jnp.dot(jnp.concatenate(lhs, 1), jnp.concatenate(rhs, 0),
                            preferred_element_type=F32)
                t = t + acc[b, :, c * 128:(c + 1) * 128]
                if stage == OC:
                    out_ref[b, :, c * 128:(c + 1) * 128] = t.astype(out_ref.dtype)
                else:
                    acc[b, :, c * 128:(c + 1) * 128] = t

    def cast_x(b):
        load_x[b].wait()
        for k in range(4):
            xs[b, k] = _pack(x_f32[b, :, k * 128:(k + 1) * 128])

    for cp in load_wq:
        cp.start()
    rx[:, :, RAW:END] = jnp.zeros((6, 2, END - RAW, 128), I32)

    barrier = pltpu.get_barrier_semaphore()

    @pl.when(me != 2)
    def _():
        for n in nbr:
            pl.semaphore_signal(barrier, inc=1, device_id=(n,), device_id_type=MESH)

    load_x[0].start()
    load_kv(0)
    load_wo.start()
    load_x[1].start()
    load_kv(1)

    @pl.when((me & 1) == 1)
    def _():
        pl.semaphore_wait(barrier, 1)

    @pl.when(me == 2)
    def _():
        pl.semaphore_wait(barrier, 2)
        for n in nbr:
            pl.semaphore_signal(go_sem, inc=1, device_id=(n,), device_id_type=MESH)

    unheard = ((me == 0) | (me == 3), (me == 0) | (me == 1))
    lead = BITS + _WQ_ROWS[1] // 4
    for cp, a, b in zip(load_wq, _WQ_ROWS, _WQ_ROWS[1:]):
        cp.wait()
        for p in range(2):
            own[p, a // 2:b // 2] = _pack(wq_f32[a:b, p * 128:(p + 1) * 128])
            put_bits(p, a // 2, b // 2)
        for d in range(2):
            @pl.when(jnp.logical_not(unheard[d]))
            def _():
                copy(QA, d, BITS + a // 4, BITS + b // 4, bits_sem(QA, 0, 8)).start()
                if a == 0:
                    copy(QB, d, BITS, lead, bits_sem(QB, 0, 8)).start()
    put_code(0)
    put_code(1)
    load_kv(2, 3)

    @pl.when(me == 0)
    def _():
        pl.semaphore_wait(barrier, 2)

    @pl.when((me & 1) == 1)
    def _():
        pl.semaphore_wait(go_sem, 1)

    for d in range(2):
        pl.when(unheard[d])(copy(QA, d, BITS, RAW, bits_sem(QA, 0, 8)).start)
    send_code(QA)
    send_code(QB)
    for d in range(2):
        copy(QB, d, lead, RAW, bits_sem(QB, 0, 8)).start()
        pl.when(unheard[d])(copy(QB, d, BITS, lead, bits_sem(QB, 0, 8)).start)

    cast_x(0)
    query(0, 1)

    wait_kv(0)
    softmax(0, 1)
    context(0, 1)
    load_kv(4)

    load_wo.wait()
    for h in range(2):
        for c in range(4):
            for p in range(2):
                r = p * 128 + h * BLK
                own[2 + h, 64 * c + 32 * p:64 * c + 32 * p + 32] = _pack(
                    wo_f32[r:r + BLK, c * 128:(c + 1) * 128])
        put_bits(2 + h, 0, 256)
    put_code(2)
    put_code(3)
    load_kv(5)
    send_code(OA)

    cast_x(1)
    query(2, 3)

    recv_code(QA)
    send_code(QC)
    code = read_code(QA)
    wait_kv(1)
    recv_bits((QA, 0, 8))
    send_bits((OA, 0, 2), (QC, 0, 8))
    send_code(OB)
    send_bits((OA, 2, 8), (OB, 0, 6))
    decode(QA, code)
    project_own(0, 0)
    softmax(2, 3)
    project_own(0, 1, 2, 3)
    context(2, 3)
    load_kv(6, 7)

    recv_code(QB)
    code = read_code(QB)
    wait_kv(2)
    recv_raw(QA)
    project_own(1, 0)
    query(4, 5)
    softmax(4)
    query(6, 7)
    softmax(5)
    context(4)
    project_own(1, 1, 2)
    context(5)
    project_own(1, 3)
    decode(QB, code)

    recv_code(QC)
    code = read_code(QC)
    wait_kv(3, 4)
    recv_bits((QB, 0, 8))
    recv_raw(QB)
    query(8, 9)
    softmax(6, 7)
    query(10)
    softmax(9, 8)
    query(11)
    context(7, 8, 9, 6)
    decode(QC, code)

    recv_code(OA)
    code = read_code(OA)
    wait_kv(5, 6)
    recv_bits((QC, 0, 8), (OA, 0, 2))
    recv_raw(QC)
    send_code(OC)
    send_bits((OB, 6, 8), (OC, 0, 2))
    query(12)
    softmax(10, 11)
    query(13)
    softmax(12)
    context(11)
    softmax(13)
    query(14, 15)
    context(12, 13, 10)
    decode(OA, code)

    recv_code(OB)
    code = read_code(OB)
    wait_kv(7)
    recv_bits((OA, 2, 8))
    recv_raw(OA)
    send_bits((OC, 2, 4), (OC, 4, 6), (OC, 6, 8))
    project(OA, 0, 1)
    softmax(14, 15)
    project(OA, 2)
    context(14)
    project(OA, 3)
    context(15)
    decode(OB, code)

    recv_code(OC)
    code = read_code(OC)
    recv_bits((OB, 0, 6))
    recv_raw(OB)
    project(OB, 0, 1, 2)
    decode(OC, code)

    recv_bits((OB, 6, 8), (OC, 0, 2))
    recv_raw(OC)
    for sent, cp in raw_sends:
        pl.when(sent)(cp.wait_send)
    project(OB, 3)
    project(OC, 0)
    for c in (1, 2, 3):
        recv_bits((OC, 2 * c, 2 * c + 2))
        project(OC, c)

    r = rx.at[:, :, CODE:RAW]
    pltpu.make_async_copy(r, r, send_sem.at[0]).wait()


def pallas_dist_sparse_attn_causalblk_htp_bs_b2_sq256_skv256_hq4_dh64_kernel(
    x: jax.Array,
    Wq: jax.Array,
    K_ext: jax.Array,
    V_ext: jax.Array,
    Wo: jax.Array,
):
    kt = jnp.transpose(K_ext, (0, 2, 3, 1)).reshape(8, 1024, SEQ)
    vt = jnp.transpose(V_ext, (0, 2, 3, 1)).reshape(8, 1024, SEQ)
    return pl.pallas_call(
        _body,
        out_shape=jax.ShapeDtypeStruct((NB, SEQ, D_MODEL), BF16),
        in_specs=[pl.BlockSpec(memory_space=pltpu.HBM)] * 5,
        out_specs=pl.BlockSpec(memory_space=pltpu.VMEM),
        scratch_shapes=[
            pltpu.VMEM((NB, SEQ, D_MODEL), F32),
            pltpu.VMEM((D_MODEL, 256), F32),
            pltpu.VMEM((256, D_MODEL), F32),
            pltpu.VMEM((16, 2, 128, SEQ), F32),
            pltpu.VMEM((NB, 4, SEQ // 2, 128), I32),
            pltpu.VMEM((4, 256, 128), I32),
            pltpu.VMEM((4, END, 128), I32),
            pltpu.VMEM((6, 2, END, 128), I32),
            pltpu.VMEM((4, 2, NB, SEQ // 2, 128), I32),
            pltpu.VMEM((NB, SEQ, D_MODEL), F32),
            pltpu.SemaphoreType.DMA((_N_WQ + 11,)),
            pltpu.SemaphoreType.DMA((13,)),
            pltpu.SemaphoreType.DMA((18 + len(_PIECES),)),
            pltpu.SemaphoreType.REGULAR,
        ],
        compiler_params=pltpu.CompilerParams(
            collective_id=0,
            vmem_limit_bytes=48 << 20,
            disable_bounds_checks=True,
            disable_semaphore_checks=True,
        ),
    )(x, Wq, kt, vt, Wo)
```

```python
import math

import jax
import jax.numpy as jnp
from jax import lax
from jax.experimental import pallas as pl
from jax.experimental.pallas import tpu as pltpu

BF16, F32, I32 = jnp.bfloat16, jnp.float32, jnp.int32
MESH = pl.DeviceIdType.MESH
NB, SEQ, D_MODEL = 2, 256, 512
BLK = 64
NBLK = SEQ // BLK
SCALE = 0.125 * math.log2(math.e)

CODE, PAD, BITS, RAW, END = 0, 45, 48, 176, 264
_srl = lax.shift_right_logical
_EXP = 0x7F807F80
_HEAD, _HOME, _TAIL = 9, 96, 192
_TOP_BIAS, _RANK_BIAS = 1690, 1368
_WORDS = [5] * 4 + [4] * 4 + [3] * 4 + [2] * 3 + [1]


def _bytes(b):
    v = b * 0x01010101
    return v - (1 << 32) if v >> 31 else v


def _splat(v):
    v = v | (v << 8)
    return v | (v << 16)


def _sign_mantissa(w0, w1):
    return (w0 & ~_EXP) | (((w1 << 8) | _srl(w1, 24)) & _EXP)


def _exponents(w0, w1):
    return (_srl(w0, 7) & 0x00FF00FF) | ((w1 << 1) & ~0x00FF00FF)


def _join(sm, e):
    return [(sm & ~_EXP) | ((e << 7) & _EXP),
            ((_srl(sm, 8) | (sm << 24)) & ~_EXP) | (_srl(e, 1) & _EXP)]


def _below(v, k, on):
    return _srl(_bytes(127 + (1 << k)) - v, 7) & on


def _rot_up(v, k, on):
    t = _below(v, k, on)
    return (v + t) & ~(t << k)


def _rot_down(v, k, on):
    t = _below(v, k, on)
    return ((v | (t << k)) - t) & ~(t << k)


def _reverse_bits(v):
    for n, m in ((1, 0x55555555), (2, 0x33333333), (4, 0x0F0F0F0F), (8, 0x00FF00FF)):
        v = ((v & m) << n) | (_srl(v, n) & m)
    return (v << 16) | _srl(v, 16)


def _count_ones(v):
    c2 = v - (_srl(v, 1) & 0x55555555)
    c4 = (c2 & 0x33333333) + (_srl(c2, 2) & 0x33333333)
    c8 = (c4 + _srl(c4, 4)) & 0x0F0F0F0F
    c16 = (c8 + _srl(c8, 8)) & 0x00FF00FF
    return v, c2, c4, c8, c16, (c16 + _srl(c16, 16)) & 63


def _scan_rows(op, v, row):
    for n in (1, 2, 4):
        v = jnp.where(row >= n, op(v, pltpu.roll(v, n, 0)), v)
    return v


def _over_rows(op, v):
    for n in (1, 2, 4):
        v = op(v, pltpu.roll(v, n, 0))
    return v


def _mean_exponent(w):
    tot = _over_rows(jnp.add, sum(_srl(v, 7) & 0x00FF00FF for v in w))
    tot = (tot & 0xFFFF) + _srl(tot, 16)
    return _srl(sum((pltpu.roll(tot, n, 1) for n in range(16, 128, 16)), tot), 1)


def _max_power(w, big):
    for v in w:
        big = jnp.maximum(big, jnp.maximum(pltpu.bitcast((v << 16) & 0x7F800000, F32),
                                           pltpu.bitcast(v & 0x7F800000, F32)))
    return big


def _encode(w, tot, big):
    row = lax.broadcasted_iota(I32, (8, 128), 0)

    big = _srl(pltpu.bitcast(_over_rows(jnp.maximum, big), I32), 23)
    top = jnp.minimum(jnp.maximum(big, _srl(tot + _TOP_BIAS, 9)), 255)
    ranking = jnp.where((top << 9) - tot > _RANK_BIAS, 1, 0)
    top4, ranking4 = _splat(top), _splat(ranking)

    e = [_exponents(w[2 * k], w[2 * k + 1]) for k in range(16)]
    odd, bad, groups = [0, 0], 0, []
    for k in range(16):
        d = top4 - e[k]
        bad |= d & _bytes(0xC0)
        u = _rot_down(_rot_down(d, 3, _bytes(1)), 2, ranking4)
        odd[k // 8] |= (u & _bytes(1)) << (k % 8)
        stop = _srl(u, 1) & _bytes(31)
        stop = stop + 0x01010100
        stop = stop + (stop << 8)
        stop = stop + (stop << 16)
        bits = 0
        for b in range(4):
            bits |= 1 << (_srl(stop, 8 * b) & 31)
        n = _srl(stop, 24) + 1
        bad |= n & ~31
        groups.append((bits, n & 31))

    stream, total = [groups[15][0]], groups[15][1]
    for k in range(14, -1, -1):
        bits, n = groups[k]
        if _WORDS[k] > _WORDS[k + 1]:
            bad |= (32 * _WORDS[k + 1] - total) & ~255
        back = (32 - n) & 31
        stream = ([(stream[0] << n) | bits]
                  + [(a << n) | _srl(b, back) for a, b in zip(stream[1:], stream)]
                  + [_srl(stream[-1], back)])[:_WORDS[k]]
        total = total + n

    over = total - _HOME
    off = _scan_rows(jnp.add, over, row) - over + _HEAD
    off = off - jnp.minimum(_scan_rows(jnp.minimum, off, row), 0)
    end = off + over
    n = off & 31
    x = ([stream[0] << n]
         + [(a << n) | _srl(_srl(b, 1), 31 - n) for a, b in zip(stream[1:], stream)]
         + [_srl(_srl(stream[-1], 1), 31 - n)])
    for step in (1, 2, 4):
        move = (off & (32 * step)) != 0
        x = [jnp.where(move, a, b) for a, b in zip([0] * step + x, x + [0] * step)][:9]
    home, tail = [], 0
    for j in range(3):
        h, t = x[j], 0
        for m in (1, 2):
            r = pltpu.roll(x[j + 3 * m], m, 0)
            h, t = h | jnp.where(row < m, 0, r), t | jnp.where(row < m, r, 0)
        home.append(h)
        tail |= pltpu.roll(t, 2 * j, 0) if j else t
    home[0] |= jnp.where(row == 0, top | (ranking << 8), 0)
    tail |= jnp.where(row == 3, _reverse_bits(pltpu.roll(pltpu.roll(tail, 6, 0), 64, 1)), 0)
    misfit = ((bad != 0) | (total > 32 * _WORDS[0]) | (end > _TAIL)
              | ((row == 7) & (end + pltpu.roll(end, 64, 1) > 2 * (_TAIL - 32)))
              | ((row == 0) & (tail == -1)))
    return e, odd + home + [tail], jnp.max(jnp.where(misfit, 1.0, 0.0)) > 0.5


def _decode(code):
    row = lax.broadcasted_iota(I32, (8, 128), 0)
    odd, home, tail = code[:2], code[2:5], code[5]
    head = jnp.broadcast_to(home[0][:1], (8, 128))
    top4, ranking4 = _splat(head & 255), _splat(_srl(head, 8) & 1)
    home[0] = jnp.where(row == 0, home[0] & -(1 << _HEAD), home[0])
    last = _reverse_bits(pltpu.roll(pltpu.roll(tail, 64, 1), 2, 0))

    def from_home(home, tail, n):
        out = list(home)
        for i in range(3, n):
            m, j = divmod(i, 3)
            t = pltpu.roll(tail, 8 - 2 * j, 0) if j else tail
            out.append(pltpu.roll(jnp.where(row < m, t, home[j]), 8 - m, 0))
        return out

    x = from_home(home, jnp.where(row == 5, last, tail), 9)
    ones = from_home([_count_ones(v)[5] for v in home], _count_ones(tail)[5], 6)
    mine = ones[0] + ones[1] + ones[2]
    skip = (row << 6) - _scan_rows(jnp.add, mine, row) + mine
    for step in (4, 2, 1):
        n = sum(ones[1:step], ones[0])
        move = skip > n
        skip = jnp.where(move, skip - n, skip)
        x = [jnp.where(move, x[min(i + step, len(x) - 1)], x[i]) for i in range(5 + step)]
        ones = [jnp.where(move, ones[min(i + step, len(ones) - 1)], ones[i])
                for i in range(step - 1)]
    counts, at = _count_ones(x[0]), jnp.zeros((8, 128), I32)
    for k in (4, 3, 2, 1, 0):
        n = _srl(counts[k], at) & ((1 << (1 << k)) - 1)
        move = skip > n
        skip, at = jnp.where(move, skip - n, skip), jnp.where(move, at + (1 << k), at)
    at = jnp.where(row == 0, _HEAD - 1, at)
    stream = [jnp.where((skip > 0) | (row == 0), _srl(_srl(a, at), 1) | (b << (31 - at)), a)
              for a, b in zip(x, x[1:])]

    e = []
    for k in range(16):
        v, stop = stream[0], 0
        for b in range(4):
            rest = v & (v - 1)
            f = pltpu.bitcast((v - rest).astype(F32), I32)
            stop |= _srl(f, 23 - 8 * b) if b < 3 else f << 1
            v = rest
        u = ((stop - (stop << 8) - 0x0101017F) << 1) | (_srl(odd[k // 8], k % 8) & _bytes(1))
        e.append(top4 - _rot_up(_rot_up(u, 2, ranking4), 3, _bytes(1)))
        if k < 15:
            n = (_srl(f, 23) + 2) & 31
            back = (32 - n) & 31
            stream = ([_srl(a, n) | (b << back) for a, b in zip(stream, stream[1:])]
                      + [_srl(stream[-1], n)])[:_WORDS[k + 1]]
    return e


QA, QB, QC, OA, OB, OC = range(6)
_WQ_ROWS = (0, 32, 64, 128, 192, 256, 384, 512)
_PIECES = ((QA, 0, 8), (QB, 0, 8), (QC, 0, 8), (OA, 0, 1), (OA, 1, 4), (OA, 4, 8),
           (OB, 0, 6), (OB, 6, 8), (OC, 0, 2), (OC, 2, 4), (OC, 4, 6), (OC, 6, 8))
_N_WQ = len(_WQ_ROWS) - 1


def _pack(v):
    return pltpu.bitcast(v.astype(BF16), I32)


def _bf16(v):
    return pltpu.bitcast(v, BF16)


def _tiles(v):
    return [v[i:i + 8] for i in range(0, v.shape[0], 8)]


def _unit(u):
    g, r = divmod(u, 4)
    return (g, r % 2, r // 2) if g == 0 else (g, r // 2, r % 2)


def _body(x_hbm, wq_hbm, kt_hbm, vt_hbm, wo_hbm, out_ref,
          x_f32, wq_f32, wo_f32, kv_f32, xs, own, tx, rx, exps, ctx, acc,
          load_sem, send_sem, recv_sem, go_sem):
    me = lax.axis_index("i")
    nbr = (me ^ 1, me ^ 3)
    head_owner = ((me, me), (nbr[0], nbr[1]), (nbr[1], nbr[0]), (me ^ 2, me ^ 2))

    load_wq = [pltpu.make_async_copy(wq_hbm.at[a:b], wq_f32.at[a:b], load_sem.at[i])
               for i, (a, b) in enumerate(zip(_WQ_ROWS, _WQ_ROWS[1:]))]
    load_x = [pltpu.make_async_copy(x_hbm.at[b], x_f32.at[b], load_sem.at[_N_WQ + b])
              for b in range(NB)]
    load_wo = pltpu.make_async_copy(wo_hbm, wo_f32, load_sem.at[_N_WQ + 2])

    def load_kv(*pairs):
        for h in pairs:
            for u in (2 * h, 2 * h + 1):
                g, p, b = _unit(u)
                rows = pl.ds(pl.multiple_of(head_owner[g][p] * 256 + p * 128, 128), 128)
                for t, src in enumerate((kt_hbm, vt_hbm)):
                    pltpu.make_async_copy(src.at[me * NB + b, rows], kv_f32.at[u, t],
                                          load_sem.at[_N_WQ + 3 + h]).start()

    def wait_kv(*pairs):
        for h in pairs:
            r = kv_f32.at[2 * h:2 * h + 2]
            pltpu.make_async_copy(r, r, load_sem.at[_N_WQ + 3 + h]).wait()

    verbatim, raw_sends = {}, []

    def route(stage, d):
        part = d if stage % 3 == 0 else 1 - d
        if stage % 3 == 2:
            return part, rx.at[stage - 2, part], (stage - 2, part)
        m = 2 * (stage // 3) + part
        return part, tx.at[m], m

    def copy(stage, d, a, b, recv, send=12):
        part, src, _ = route(stage, d)
        return pltpu.make_async_remote_copy(
            src.at[a:b], rx.at[stage, part, a:b], send_sem.at[send], recv_sem.at[recv],
            device_id=(nbr[d],), device_id_type=MESH)

    def bits_sem(*piece):
        return 18 + _PIECES.index(piece)

    def send_bits(*pieces):
        for stage, a, b in pieces:
            for d in range(2):
                copy(stage, d, BITS + 16 * a, BITS + 16 * b, bits_sem(stage, a, b)).start()

    def recv_bits(*pieces):
        for stage, a, b in pieces:
            r = rx.at[stage, :, BITS + 16 * a:BITS + 16 * b]
            pltpu.make_async_copy(r, r, recv_sem.at[bits_sem(stage, a, b)]).wait()

    def send_raw(stage):
        for d in range(2):
            part, _, key = route(stage, d)
            cp = copy(stage, d, RAW, END, 2 * stage + part, 2 * stage + part)
            pl.when(verbatim[key])(cp.start)
            raw_sends.append((verbatim[key], cp))

    def recv_raw(stage):
        for part in range(2):
            r = rx.at[stage, part, RAW:END]
            pl.when(verbatim[stage, part])(
                pltpu.make_async_copy(r, r, recv_sem.at[2 * stage + part]).wait)
        if stage % 3 == 0:
            send_raw(stage + 2)

    def send_code(stage):
        for d in range(2):
            copy(stage, d, CODE, PAD, 12 + stage, 13).start()
        if stage % 3 < 2:
            send_raw(stage)

    def recv_code(stage):
        r = rx.at[stage, :, CODE:PAD]
        pltpu.make_async_copy(r, r, recv_sem.at[12 + stage]).wait()

    mean, big = {}, {}

    def put_bits(m, a, b):
        w = _tiles(own[m, a:b])
        big[m] = _max_power(w, big.get(m, 0.0))
        if a <= 128 < b:
            mean[m] = _mean_exponent(_tiles(own[m, 0:64]))
        for k in range(len(w) // 2):
            r = BITS + a // 2 + 8 * k
            tx[m, r:r + 8] = _sign_mantissa(w[2 * k], w[2 * k + 1])

    def put_code(m):
        e, code, verbatim[m] = _encode(_tiles(own[m]), mean[m], big[m])
        tx[m, CODE:BITS] = jnp.concatenate(
            [jnp.where(verbatim[m], a, b) for a, b in zip(e[:5] + [-1], code)], 0)
        tx[m, RAW:END] = jnp.concatenate(e[5:], 0)

    due = []

    def decode(stage, *parts):
        for part in parts:
            code = _tiles(rx[stage, part, CODE:BITS])
            verbatim[stage, part] = code[5][0, 0] == -1
            for k, e in enumerate(_decode(code)):
                exps[stage, part, k] = e
            e = [exps[stage, part, k] for k in range(16)]
            due.append(jnp.minimum(jnp.abs(sum(e[1:], e[0]).astype(F32)), 0.0))

    def operand(v):
        while due:
            v = jnp.concatenate([v[:8] + due.pop().astype(v.dtype), v[8:]], 0)
        return v

    def received(stage, part, k0, k1):
        msg = rx.at[stage, part]
        marker = jnp.broadcast_to(msg[BITS - 8:BITS - 7], (8, 128)) == -1
        out = []
        for k in range(k0, k1):
            r = CODE + 8 * k if k < 5 else RAW + 8 * (k - 5)
            e = jnp.where(marker, msg[r:r + 8], exps[stage, part, k])
            out += _join(msg[BITS + 8 * k:BITS + 8 * k + 8], e)
        return _bf16(jnp.concatenate(out, 0))

    first = lax.broadcasted_iota(I32, (BLK, 128), 1) < BLK
    wq, q, prob, inv = {}, {}, {}, {}

    def block_diag(u, t):
        out = []
        for h in range(2):
            v = operand(kv_f32[u, t, :, h * 128:(h + 1) * 128])
            h0, h1 = v[:BLK], v[BLK:]
            r = pltpu.roll(jnp.where(first, h1, h0), BLK, 1)
            for a, b in ((h0, r), (r, h1)):
                out.append(jnp.concatenate(
                    [jnp.where(first, a, 0.0), jnp.where(first, 0.0, b)], 0).astype(BF16))
        return out

    def query(*units):
        for u in units:
            g, p, b = _unit(u)
            if g == 0:
                wq[g, p] = _bf16(own[p])
            elif b == 0:
                wq[g, p] = received(g - 1, p, 0, 16)
            lhs = jnp.concatenate([_bf16(operand(xs[b, k])) for k in range(4)], 1)
            q[u] = jnp.dot(lhs, wq[g, p], preferred_element_type=F32)

    def softmax(*units):
        for u in units:
            k = block_diag(u, 0)
            s = [jnp.dot(q[u][j * BLK:].astype(BF16), k[j], preferred_element_type=F32)
                 for j in range(NBLK)]
            w, inv[u] = [[] for _ in range(NBLK)], []
            for i in range(NBLK):
                blocks = [s[j][(i - j) * BLK:(i - j + 1) * BLK] for j in range(i + 1)]
                m = blocks[0]
                for t in blocks[1:]:
                    m = jnp.maximum(m, t)
                m = jnp.where(first,
                              jnp.max(jnp.where(first, m, -jnp.inf), axis=1, keepdims=True),
                              jnp.max(jnp.where(first, -jnp.inf, m), axis=1, keepdims=True))
                tot = None
                for j in range(i + 1):
                    e = jnp.exp2(blocks[j] - m)
                    tot = e if tot is None else tot + e
                    w[j].append(e)
                tot = jnp.where(first,
                                jnp.sum(jnp.where(first, tot, 0.0), axis=1, keepdims=True),
                                jnp.sum(jnp.where(first, 0.0, tot), axis=1, keepdims=True))
                inv[u].append(pl.reciprocal(tot, approx=True))
            prob[u] = [jnp.concatenate(t, 0).astype(BF16) for t in w]

    def context(*units):
        for u in units:
            g, p, b = _unit(u)
            v = block_diag(u, 1)
            o = [lax.dot_general(prob[u][j], v[j], (((1,), (1,)), ((), ())),
                                 preferred_element_type=F32) for j in range(NBLK)]
            for i in range(NBLK):
                t = o[0][i * BLK:(i + 1) * BLK]
                for j in range(1, i + 1):
                    t = t + o[j][(i - j) * BLK:(i - j + 1) * BLK]
                ctx[g, p, b, i * 32:(i + 1) * 32] = _pack(t * inv[u][i])

    def project_own(b, *cols):
        for c in cols:
            rhs = [_bf16(own[2 + h, 64 * c + 32 * p:64 * c + 32 * p + 32])
                   for p in range(2) for h in range(2)]
            for r in (0, 128):
                lhs = [_bf16(operand(ctx[0, p, b, r // 2:r // 2 + 64])) for p in range(2)]
                acc[b, r:r + 128, c * 128:(c + 1) * 128] = jnp.dot(
                    jnp.concatenate(lhs, 1), jnp.concatenate(rhs, 0), preferred_element_type=F32)

    def project(stage, *cols):
        def heads(p, b):
            if stage == OC:
                return ctx[3, p, b]
            g0, g1 = (1 + p, 2 - p) if stage == OA else (2 - p, 1 + p)
            return jnp.where(lax.broadcasted_iota(I32, (SEQ // 2, 128), 1) < BLK,
                             ctx[g0, p, b], ctx[g1, p, b])

        for c in cols:
            rhs = [received(stage, h, 4 * c + 2 * p, 4 * c + 2 * p + 2)
                   for p in range(2) for h in range(2)]
            for b in range(NB):
                lhs = [heads(p, b) for p in range(2)]
                lhs = [_bf16(v if stage == OB else operand(v)) for v in lhs]
                t = jnp.dot(jnp.concatenate(lhs, 1), jnp.concatenate(rhs, 0),
                            preferred_element_type=F32)
                t = t + operand(acc[b, :, c * 128:(c + 1) * 128])
                if stage == OC:
                    out_ref[b, :, c * 128:(c + 1) * 128] = t.astype(out_ref.dtype)
                else:
                    acc[b, :, c * 128:(c + 1) * 128] = t

    def cast_x(b):
        load_x[b].wait()
        for k in range(4):
            xs[b, k] = _pack(x_f32[b, :, k * 128:(k + 1) * 128] * SCALE)

    for cp in load_wq:
        cp.start()
    for a, b in ((BITS - 8, BITS), (RAW, END)):
        rx[:, :, a:b] = jnp.zeros((6, 2, b - a, 128), I32)

    barrier = pltpu.get_barrier_semaphore()

    @pl.when(me != 2)
    def _():
        for n in nbr:
            pl.semaphore_signal(barrier, inc=1, device_id=(n,), device_id_type=MESH)

    load_x[0].start()
    load_kv(0)
    load_wo.start()
    load_x[1].start()
    load_kv(1)

    @pl.when((me & 1) == 1)
    def _():
        pl.semaphore_wait(barrier, 1)

    @pl.when(me == 2)
    def _():
        pl.semaphore_wait(barrier, 2)
        for n in nbr:
            pl.semaphore_signal(go_sem, inc=1, device_id=(n,), device_id_type=MESH)

    unheard = ((me == 0) | (me == 3), (me == 0) | (me == 1))
    lead = BITS + _WQ_ROWS[1] // 4
    for cp, a, b in zip(load_wq, _WQ_ROWS, _WQ_ROWS[1:]):
        cp.wait()
        for p in range(2):
            own[p, a // 2:b // 2] = _pack(wq_f32[a:b, p * 128:(p + 1) * 128])
            put_bits(p, a // 2, b // 2)
        for d in range(2):
            @pl.when(jnp.logical_not(unheard[d]))
            def _():
                copy(QA, d, BITS + a // 4, BITS + b // 4, bits_sem(QA, 0, 8)).start()
                if a == 0:
                    copy(QB, d, BITS, lead, bits_sem(QB, 0, 8)).start()
    put_code(0)
    put_code(1)
    load_kv(2, 3)

    @pl.when(me == 0)
    def _():
        pl.semaphore_wait(barrier, 2)

    @pl.when((me & 1) == 1)
    def _():
        pl.semaphore_wait(go_sem, 1)

    for d in range(2):
        pl.when(unheard[d])(copy(QA, d, BITS, RAW, bits_sem(QA, 0, 8)).start)
    send_code(QA)
    send_code(QB)
    for d in range(2):
        copy(QB, d, lead, RAW, bits_sem(QB, 0, 8)).start()
        pl.when(unheard[d])(copy(QB, d, BITS, lead, bits_sem(QB, 0, 8)).start)

    cast_x(0)
    query(0, 1)

    wait_kv(0)
    softmax(0, 1)
    context(0, 1)
    load_kv(4)

    load_wo.wait()
    for h in range(2):
        for c in range(4):
            for p in range(2):
                r = p * 128 + h * BLK
                own[2 + h, 64 * c + 32 * p:64 * c + 32 * p + 32] = _pack(
                    wo_f32[r:r + BLK, c * 128:(c + 1) * 128])
        put_bits(2 + h, 0, 256)
    send_bits((OA, 0, 1))
    put_code(2)
    put_code(3)
    project_own(0, 0, 1, 2, 3)
    load_kv(5)

    def pass_on_code():
        recv_code(QA)
        send_code(QC)

    pl.when(me != 0)(pass_on_code)
    send_code(OA)

    cast_x(1)
    query(2, 3)

    pl.when(me == 0)(pass_on_code)
    wait_kv(1)
    recv_bits((QA, 0, 8))
    send_bits((QC, 0, 8), (OA, 1, 4), (OA, 4, 8))
    send_code(OB)
    softmax(2, 3)
    context(2, 3)
    decode(QA, 0)
    project_own(1, 0)
    decode(QA, 1)
    project_own(1, 1)
    load_kv(6, 7)

    recv_code(QB)
    wait_kv(2)
    recv_raw(QA)
    project_own(1, 2)
    query(4, 5)
    softmax(4, 5)
    decode(QB, 0)
    query(6)
    context(4)
    query(7)
    decode(QB, 1)
    context(5)
    project_own(1, 3)

    recv_code(QC)
    wait_kv(3, 4)
    recv_bits((QB, 0, 8))
    recv_raw(QB)
    send_bits((OB, 0, 6))
    query(8, 9)
    softmax(6)
    query(10)
    softmax(7, 9, 8)
    context(7)
    decode(QC, 0)
    query(11)
    decode(QC, 1)
    context(8, 6, 9)

    recv_code(OA)
    send_code(OC)
    send_bits((OB, 6, 8))
    wait_kv(5, 6)
    recv_bits((QC, 0, 8))
    recv_raw(QC)

    def pass_on_bits():
        recv_bits((OA, 0, 1), (OA, 1, 4))
        send_bits((OC, 0, 2), (OC, 2, 4))

    pl.when((me & 1) == 1)(pass_on_bits)
    query(12)
    softmax(11)
    query(13)
    softmax(12)
    context(11)
    softmax(10)
    decode(OA, 0)
    query(14)
    context(10, 12)
    softmax(13)
    decode(OA, 1)
    query(15)
    context(13)

    pl.when((me & 1) == 0)(pass_on_bits)
    recv_bits((OA, 4, 8))
    send_bits((OC, 4, 6), (OC, 6, 8))
    recv_code(OB)
    wait_kv(7)
    recv_raw(OA)
    project(OA, 0, 1)
    softmax(14)
    project(OA, 2)
    softmax(15)
    decode(OB, 0)
    project(OA, 3)
    decode(OB, 1)
    context(15, 14)

    recv_code(OC)
    recv_bits((OB, 0, 6))
    recv_raw(OB)
    project(OB, 0, 1)
    decode(OC, 0, 1)
    project(OB, 2)

    recv_bits((OB, 6, 8), (OC, 0, 2))
    recv_raw(OC)
    for sent, cp in raw_sends:
        pl.when(sent)(cp.wait_send)
    r = rx.at[:, :, CODE:PAD]
    pltpu.make_async_copy(r, r, send_sem.at[13]).wait()
    project(OB, 3)
    project(OC, 0)
    for c in (1, 2, 3):
        recv_bits((OC, 2 * c, 2 * c + 2))
        project(OC, c)

    r = rx.at[:, :, BITS:RAW]
    pltpu.make_async_copy(r, r, send_sem.at[12]).wait()


def pallas_dist_sparse_attn_causalblk_htp_bs_b2_sq256_skv256_hq4_dh64_kernel(
    x: jax.Array,
    Wq: jax.Array,
    K_ext: jax.Array,
    V_ext: jax.Array,
    Wo: jax.Array,
):
    kt = jnp.transpose(K_ext, (0, 2, 3, 1)).reshape(8, 1024, SEQ)
    vt = jnp.transpose(V_ext, (0, 2, 3, 1)).reshape(8, 1024, SEQ)
    return pl.pallas_call(
        _body,
        out_shape=jax.ShapeDtypeStruct((NB, SEQ, D_MODEL), BF16),
        in_specs=[pl.BlockSpec(memory_space=pltpu.HBM)] * 5,
        out_specs=pl.BlockSpec(memory_space=pltpu.VMEM),
        scratch_shapes=[
            pltpu.VMEM((NB, SEQ, D_MODEL), F32),
            pltpu.VMEM((D_MODEL, 256), F32),
            pltpu.VMEM((256, D_MODEL), F32),
            pltpu.VMEM((16, 2, 128, SEQ), F32),
            pltpu.VMEM((NB, 4, SEQ // 2, 128), I32),
            pltpu.VMEM((4, 256, 128), I32),
            pltpu.VMEM((4, END, 128), I32),
            pltpu.VMEM((6, 2, END, 128), I32),
            pltpu.VMEM((6, 2, 16, 8, 128), I32),
            pltpu.VMEM((4, 2, NB, SEQ // 2, 128), I32),
            pltpu.VMEM((NB, SEQ, D_MODEL), F32),
            pltpu.SemaphoreType.DMA((_N_WQ + 11,)),
            pltpu.SemaphoreType.DMA((14,)),
            pltpu.SemaphoreType.DMA((18 + len(_PIECES),)),
            pltpu.SemaphoreType.REGULAR,
        ],
        compiler_params=pltpu.CompilerParams(
            collective_id=0,
            vmem_limit_bytes=48 << 20,
            disable_bounds_checks=True,
            disable_semaphore_checks=True,
        ),
    )(x, Wq, kt, vt, Wo)
```
